```python
import numpy as np

kernel_name = "dist_argmax_global_i_m8192_n1024"

def setup_inputs():
    return {"x": np.random.randn(32768, 1024).astype(np.float32)}

def reference(x: np.ndarray) -> np.ndarray:
    idx = np.argmax(x, axis=0).astype(np.float32)
    val = np.max(x, axis=0)
    return np.stack([val, idx], axis=0)
```

```python
import jax
import jax.numpy as jnp
from jax import lax
from jax.experimental import pallas as pl
from jax.experimental.pallas import tpu as pltpu

NDEV = 4
MESH = pl.DeviceIdType.MESH
SUB, LANE = 8, 128

FULL = (5472, 1408)
REMOTE = (400, 64)
LATE = (320, 64)
UNROLL = 4
STATIC_GROUPS = 8
BLOCK_ORDER = (0, 4, 1, 5, 2, 6, 3, 7)


def _offsets(sizes):
    offs = [0]
    for s in sizes:
        offs.append(offs[-1] + s)
    return offs


def _lexmerge(a, b):
    (av, ai), (bv, bi) = a, b
    take = jnp.logical_or(bv > av, jnp.logical_and(bv == av, bi < ai))
    return jnp.where(take, bv, av), jnp.where(take, bi, ai)


def _fold(a, b):
    take = b[0] > a[0]
    return jnp.where(take, b[0], a[0]), jnp.where(take, b[1], a[1])


def _butterfly(tiles):
    sub = lax.broadcasted_iota(jnp.int32, (SUB, LANE), 0)
    for half in (4, 2, 1):
        lo = (sub & half) == 0
        n = len(tiles) // 2

        def kept(j, k):
            return jnp.where(lo, tiles[j][k], tiles[j + n][k])

        def moved(j, k):
            if half == 4:
                return pltpu.roll(jnp.where(lo, tiles[j + n][k], tiles[j][k]), 4, 0)
            return jnp.where(lo, pltpu.roll(tiles[j][k], SUB - half, 0),
                             pltpu.roll(tiles[j + n][k], half, 0))

        tiles = [_lexmerge((kept(j, 0), kept(j, 1)), (moved(j, 0), moved(j, 1)))
                 for j in range(n)]
    return tiles[0]


def pallas_dist_argmax_global_i_m8192_n1024_kernel(x: jax.Array):
    m_rows, n_cols = x.shape
    foffs, roffs, loffs = _offsets(FULL), _offsets(REMOTE), _offsets(LATE)
    n_full, n_remote, n_late = foffs[-1], roffs[-1], loffs[-1]
    nf, nr, nl = len(FULL), len(REMOTE), len(LATE)
    n_local = n_full + n_late
    assert n_local + 2 * n_remote == m_rows and n_cols == SUB * LANE
    groups = m_rows // SUB

    def body(x_hbm, out_ref, buf, strip, rbuf, acc_v, acc_i, dense, head, final,
             full_sems, wide_sems, strip_sems, raw_send_sems, raw_recv_sems,
             send_sems, recv_sems, far_sem):
        def load_full(c):
            rows = pl.ds(foffs[c], FULL[c])
            return pltpu.make_async_copy(x_hbm.at[rows, :], buf.at[rows, :], full_sems.at[c])

        def load_wide(c):
            rows = pl.ds(n_full + loffs[c], LATE[c])
            cols = pl.ds(LANE, n_cols - LANE)
            return pltpu.make_async_copy(x_hbm.at[rows, cols], buf.at[rows, cols], wide_sems.at[c])

        def load_strip(c):
            return pltpu.make_async_copy(
                x_hbm.at[pl.ds(n_full + loffs[c], LATE[c]), pl.ds(0, LANE)],
                strip.at[pl.ds(loffs[c], LATE[c]), :], strip_sems.at[c])

        for load, n in ((load_full, nf), (load_wide, nl), (load_strip, nl)):
            for c in range(n):
                load(c).start()

        my = lax.axis_index("i")
        left = (my + NDEV - 1) % NDEV
        right = (my + 1) % NDEV
        diag = (my + 2) % NDEV

        barrier = pltpu.get_barrier_semaphore()
        for peer in (left, right):
            pl.semaphore_signal(barrier, inc=1, device_id=(peer,), device_id_type=MESH)
        pl.semaphore_wait(barrier, 2)

        def raw(slot, p):
            return pltpu.make_async_remote_copy(
                src_ref=x_hbm.at[pl.ds(n_local + slot * n_remote + roffs[p], REMOTE[p]), :],
                dst_ref=rbuf.at[slot, pl.ds(roffs[p], REMOTE[p]), :],
                send_sem=raw_send_sems.at[slot, p], recv_sem=raw_recv_sems.at[slot, p],
                device_id=(right if slot == 0 else left,), device_id_type=MESH)

        for p in range(nr):
            for slot in range(2):
                raw(slot, p).start()
        pl.semaphore_signal(far_sem, inc=1, device_id=(right,), device_id_type=MESH)

        def scan(ref, c0, r0, r1, gbase, acc):
            width = ref.shape[-1] - c0
            cols = pl.ds(c0, width)
            g0, g1 = r0 // SUB, r1 // SUB

            def group(g):
                start = g * SUB if isinstance(g, int) else pl.multiple_of(g * SUB, SUB)
                return ref[pl.ds(start, SUB), cols], g + gbase

            def step(i, carry):
                for u in range(UNROLL):
                    carry = _fold(carry, group(i * UNROLL + u))
                return carry

            if acc is None:
                v, g = group(g0)
                acc = (v, jnp.full((SUB, width), g, jnp.int32))
                g0 += 1
            n_head = g1 - g0 if g1 - g0 <= STATIC_GROUPS else -g0 % UNROLL
            for g in range(g0, g0 + n_head):
                acc = _fold(acc, group(g))
            g0 += n_head
            n_steps = (g1 - g0) // UNROLL
            if n_steps:
                acc = lax.fori_loop(g0 // UNROLL, g0 // UNROLL + n_steps, step, acc)
            for g in range(g0 + n_steps * UNROLL, g1):
                acc = _fold(acc, group(g))
            return acc

        started = [False] * 3

        def accumulate(a, ref, r0, r1, gbase):
            acc = (acc_v[a], acc_i[a]) if started[a] else None
            acc_v[a], acc_i[a] = scan(ref, 0, r0, r1, gbase, acc)
            started[a] = True

        for k in range(max(nf, nr)):
            if k < nf:
                load_full(k).wait()
                accumulate(0, buf, foffs[k], foffs[k + 1], my * groups)
            if k < nr:
                for slot, src in ((0, left), (1, right)):
                    raw(slot, k).wait_recv()
                    accumulate(1 + slot, rbuf.at[slot], roffs[k], roffs[k + 1],
                               src * groups + (n_local + slot * n_remote) // SUB)
        bulk = (acc_v[0], acc_i[0])
        for a in (1, 2):
            bulk = _lexmerge(bulk, (acc_v[a], acc_i[a]))
        acc_v[0], acc_i[0] = bulk
        pl.semaphore_wait(far_sem, 1)

        late = None
        for c in range(nl):
            load_wide(c).wait()
            late = scan(buf, LANE, n_full + loffs[c], n_full + loffs[c + 1], my * groups, late)
        sub = lax.broadcasted_iota(jnp.int32, (SUB, LANE), 0)
        wv, wg = _lexmerge((acc_v[0, :, LANE:], acc_i[0, :, LANE:]), late)
        tiles = [(acc_v[0, :, :LANE], acc_i[0, :, :LANE] * SUB + sub)]
        tiles += [(wv[:, j * LANE:(j + 1) * LANE], wg[:, j * LANE:(j + 1) * LANE] * SUB + sub)
                  for j in range(SUB - 1)]
        bv, bi = _butterfly([tiles[b] for b in BLOCK_ORDER])
        bi = bi.astype(jnp.float32)

        def exchange(src, dst, k, peer):
            return pltpu.make_async_remote_copy(
                src_ref=src, dst_ref=dst, send_sem=send_sems.at[k], recv_sem=recv_sems.at[k],
                device_id=(peer,), device_id_type=MESH)

        dense[my, 0] = bv
        dense[my, 1] = bi
        send_dense = exchange(dense.at[my], dense.at[my], 0, diag)
        send_dense.start()

        sacc = None
        for c in range(nl):
            load_strip(c).wait()
            items = [(strip[pl.ds(g * SUB, SUB), :],
                      jnp.full((SUB, LANE), g, jnp.int32) + (my * groups + n_full // SUB))
                     for g in range(loffs[c] // SUB, loffs[c + 1] // SUB)]
            while len(items) > 1:
                items = [_fold(*items[i:i + 2]) if i + 1 < len(items) else items[i]
                         for i in range(0, len(items), 2)]
            sacc = items[0] if sacc is None else _fold(sacc, items[0])
        s = (sacc[0], sacc[1] * SUB + sub)
        for shift in (4, 2, 1):
            s = _lexmerge(s, (pltpu.roll(s[0], shift, 0), pltpu.roll(s[1], shift, 0)))
        sv, si = s[0], s[1].astype(jnp.float32)
        head[my, 0] = sv[0:1]
        head[my, 1] = si[0:1]
        send_head = exchange(head.at[my], head.at[my], 1, diag)
        send_head.start()

        hv, hi = _lexmerge((bv, bi), (sv, si))
        bv = jnp.where(sub == 0, hv, bv)
        bi = jnp.where(sub == 0, hi, bi)
        final[0] = bv
        final[1] = bi
        send_final = [exchange(final, dense.at[my], 2, right), exchange(final, dense.at[my], 3, left)]
        for cp in send_final:
            cp.start()

        for cp, src in ((send_final[0], left), (send_final[1], right), (send_dense, diag)):
            cp.wait_recv()
            bv, bi = _lexmerge((bv, bi), (dense[src, 0], dense[src, 1]))
        even = (sub & 1) == 0
        out_ref[0:SUB, :] = jnp.where(even, bv, pltpu.roll(bi, 1, 0))
        out_ref[SUB:2 * SUB, :] = jnp.where(even, pltpu.roll(bv, SUB - 1, 0), bi)
        for p in range(nr):
            for slot in range(2):
                raw(slot, p).wait_send()
        for cp in [send_dense, send_head] + send_final:
            cp.wait_send()
        send_head.wait_recv()
        hv, hi = _lexmerge((bv[0:1], bi[0:1]), (head[diag, 0], head[diag, 1]))
        out_ref[0:1, :] = hv
        out_ref[1:2, :] = hi

    out = pl.pallas_call(
        body,
        out_shape=jax.ShapeDtypeStruct((2 * SUB, LANE), jnp.float32),
        in_specs=[pl.BlockSpec(memory_space=pl.ANY)],
        out_specs=pl.BlockSpec(memory_space=pltpu.VMEM),
        scratch_shapes=[
            pltpu.VMEM((n_local, n_cols), jnp.float32),
            pltpu.VMEM((n_late, LANE), jnp.float32),
            pltpu.VMEM((2, n_remote, n_cols), jnp.float32),
            pltpu.VMEM((3, SUB, n_cols), jnp.float32),
            pltpu.VMEM((3, SUB, n_cols), jnp.int32),
            pltpu.VMEM((NDEV, 2, SUB, LANE), jnp.float32),
            pltpu.VMEM((NDEV, 2, 1, LANE), jnp.float32),
            pltpu.VMEM((2, SUB, LANE), jnp.float32),
            pltpu.SemaphoreType.DMA((nf,)),
            pltpu.SemaphoreType.DMA((nl,)),
            pltpu.SemaphoreType.DMA((nl,)),
            pltpu.SemaphoreType.DMA((2, nr)),
            pltpu.SemaphoreType.DMA((2, nr)),
            pltpu.SemaphoreType.DMA((4,)),
            pltpu.SemaphoreType.DMA((4,)),
            pltpu.SemaphoreType.REGULAR,
        ],
        compiler_params=pltpu.CompilerParams(
            collective_id=0,
            vmem_limit_bytes=64 * 1024 * 1024,
            disable_semaphore_checks=True,
            disable_bounds_checks=True,
        ),
    )(x)
    return out.reshape(SUB, 2, LANE).transpose(1, 0, 2).reshape(2, n_cols)
```

```python
import jax
import jax.numpy as jnp
from jax import lax
from jax.experimental import pallas as pl
from jax.experimental.pallas import tpu as pltpu

NDEV = 4
MESH = pl.DeviceIdType.MESH
SUB, LANE = 8, 128

FULL = (5472, 1408)
REMOTE = (400, 64)
LATE = (320, 64)
UNROLL = 4
STATIC_GROUPS = 8
BLOCK_ORDER = (0, 4, 1, 5, 2, 6, 3, 7)


def _offsets(sizes):
    offs = [0]
    for s in sizes:
        offs.append(offs[-1] + s)
    return offs


def _lexmerge(a, b):
    (av, ai), (bv, bi) = a, b
    take = jnp.logical_or(bv > av, jnp.logical_and(bv == av, bi < ai))
    return jnp.where(take, bv, av), jnp.where(take, bi, ai)


def _fold(a, b):
    take = b[0] > a[0]
    return jnp.where(take, b[0], a[0]), jnp.where(take, b[1], a[1])


def _butterfly(tiles):
    sub = lax.broadcasted_iota(jnp.int32, (SUB, LANE), 0)
    for half in (4, 2, 1):
        lo = (sub & half) == 0
        n = len(tiles) // 2

        def kept(j, k):
            return jnp.where(lo, tiles[j][k], tiles[j + n][k])

        def moved(j, k):
            if half == 4:
                return pltpu.roll(jnp.where(lo, tiles[j + n][k], tiles[j][k]), 4, 0)
            return jnp.where(lo, pltpu.roll(tiles[j][k], SUB - half, 0),
                             pltpu.roll(tiles[j + n][k], half, 0))

        tiles = [_lexmerge((kept(j, 0), kept(j, 1)), (moved(j, 0), moved(j, 1)))
                 for j in range(n)]
    return tiles[0]


def pallas_dist_argmax_global_i_m8192_n1024_kernel(x: jax.Array):
    m_rows, n_cols = x.shape
    foffs, roffs, loffs = _offsets(FULL), _offsets(REMOTE), _offsets(LATE)
    n_full, n_remote, n_late = foffs[-1], roffs[-1], loffs[-1]
    nf, nr, nl = len(FULL), len(REMOTE), len(LATE)
    n_local = n_full + n_late
    assert n_local + 2 * n_remote == m_rows and n_cols == SUB * LANE
    groups = m_rows // SUB

    def body(x_hbm, out_ref, buf, strip, rbuf, acc_v, acc_i, dense, head, final,
             load_sems, raw_send_sems, raw_recv_sems,
             send_sems, recv_sems, far_sem):
        def load_full(c):
            rows = pl.ds(foffs[c], FULL[c])
            return pltpu.make_async_copy(x_hbm.at[rows, :], buf.at[rows, :], load_sems.at[c])

        def load_wide(c):
            rows = pl.ds(n_full + loffs[c], LATE[c])
            cols = pl.ds(LANE, n_cols - LANE)
            return pltpu.make_async_copy(x_hbm.at[rows, cols], buf.at[rows, cols], load_sems.at[nf + c])

        def load_strip(c):
            return pltpu.make_async_copy(
                x_hbm.at[pl.ds(n_full + loffs[c], LATE[c]), pl.ds(0, LANE)],
                strip.at[pl.ds(loffs[c], LATE[c]), :], load_sems.at[nf + nl + c])

        for load, n in ((load_full, nf), (load_wide, nl), (load_strip, nl)):
            for c in range(n):
                load(c).start()

        my = lax.axis_index("i")
        left = (my + NDEV - 1) % NDEV
        right = (my + 1) % NDEV
        diag = (my + 2) % NDEV

        barrier = pltpu.get_barrier_semaphore()
        for peer in (left, right):
            pl.semaphore_signal(barrier, inc=1, device_id=(peer,), device_id_type=MESH)
        pl.semaphore_wait(barrier, 2)

        def raw(slot, p):
            return pltpu.make_async_remote_copy(
                src_ref=x_hbm.at[pl.ds(n_local + slot * n_remote + roffs[p], REMOTE[p]), :],
                dst_ref=rbuf.at[slot, pl.ds(roffs[p], REMOTE[p]), :],
                send_sem=raw_send_sems.at[slot, p], recv_sem=raw_recv_sems.at[slot, p],
                device_id=(right if slot == 0 else left,), device_id_type=MESH)

        for p in range(nr):
            for slot in range(2):
                raw(slot, p).start()
        pl.semaphore_signal(far_sem, inc=1, device_id=(right,), device_id_type=MESH)

        def scan(ref, c0, r0, r1, gbase, acc):
            width = ref.shape[-1] - c0
            cols = pl.ds(c0, width)
            g0, g1 = r0 // SUB, r1 // SUB

            def group(g):
                start = g * SUB if isinstance(g, int) else pl.multiple_of(g * SUB, SUB)
                return ref[pl.ds(start, SUB), cols], g + gbase

            def step(i, carry):
                for u in range(UNROLL):
                    carry = _fold(carry, group(i * UNROLL + u))
                return carry

            if acc is None:
                v, g = group(g0)
                acc = (v, jnp.full((SUB, width), g, jnp.int32))
                g0 += 1
            n_head = g1 - g0 if g1 - g0 <= STATIC_GROUPS else -g0 % UNROLL
            for g in range(g0, g0 + n_head):
                acc = _fold(acc, group(g))
            g0 += n_head
            n_steps = (g1 - g0) // UNROLL
            if n_steps:
                acc = lax.fori_loop(g0 // UNROLL, g0 // UNROLL + n_steps, step, acc)
            for g in range(g0 + n_steps * UNROLL, g1):
                acc = _fold(acc, group(g))
            return acc

        started = [False] * 3

        def accumulate(a, ref, r0, r1, gbase):
            acc = (acc_v[a], acc_i[a]) if started[a] else None
            acc_v[a], acc_i[a] = scan(ref, 0, r0, r1, gbase, acc)
            started[a] = True

        for k in range(max(nf, nr)):
            if k < nf:
                load_full(k).wait()
                accumulate(0, buf, foffs[k], foffs[k + 1], my * groups)
            if k < nr:
                for slot, src in ((0, left), (1, right)):
                    raw(slot, k).wait_recv()
                    accumulate(1 + slot, rbuf.at[slot], roffs[k], roffs[k + 1],
                               src * groups + (n_local + slot * n_remote) // SUB)
        bulk = (acc_v[0], acc_i[0])
        for a in (1, 2):
            bulk = _lexmerge(bulk, (acc_v[a], acc_i[a]))
        acc_v[0], acc_i[0] = bulk
        pl.semaphore_wait(far_sem, 1)

        late = None
        for c in range(nl):
            load_wide(c).wait()
            late = scan(buf, LANE, n_full + loffs[c], n_full + loffs[c + 1], my * groups, late)
        sub = lax.broadcasted_iota(jnp.int32, (SUB, LANE), 0)
        wv, wg = _lexmerge((acc_v[0, :, LANE:], acc_i[0, :, LANE:]), late)
        tiles = [(acc_v[0, :, :LANE], acc_i[0, :, :LANE] * SUB + sub)]
        tiles += [(wv[:, j * LANE:(j + 1) * LANE], wg[:, j * LANE:(j + 1) * LANE] * SUB + sub)
                  for j in range(SUB - 1)]
        bv, bi = _butterfly([tiles[b] for b in BLOCK_ORDER])
        bi = bi.astype(jnp.float32)

        def exchange(src, dst, k, peer):
            return pltpu.make_async_remote_copy(
                src_ref=src, dst_ref=dst, send_sem=send_sems.at[k], recv_sem=recv_sems.at[k],
                device_id=(peer,), device_id_type=MESH)

        dense[my, 0] = bv
        dense[my, 1] = bi
        send_dense = exchange(dense.at[my], dense.at[my], 0, diag)
        send_dense.start()

        sacc = None
        for c in range(nl):
            load_strip(c).wait()
            items = [(strip[pl.ds(g * SUB, SUB), :],
                      jnp.full((SUB, LANE), g, jnp.int32) + (my * groups + n_full // SUB))
                     for g in range(loffs[c] // SUB, loffs[c + 1] // SUB)]
            while len(items) > 1:
                items = [_fold(*items[i:i + 2]) if i + 1 < len(items) else items[i]
                         for i in range(0, len(items), 2)]
            sacc = items[0] if sacc is None else _fold(sacc, items[0])
        s = (sacc[0], sacc[1] * SUB + sub)
        for shift in (4, 2, 1):
            s = _lexmerge(s, (pltpu.roll(s[0], shift, 0), pltpu.roll(s[1], shift, 0)))
        sv, si = s[0], s[1].astype(jnp.float32)
        head[my, 0] = sv[0:1]
        head[my, 1] = si[0:1]
        send_head = exchange(head.at[my], head.at[my], 1, diag)
        send_head.start()

        hv, hi = _lexmerge((bv, bi), (sv, si))
        bv = jnp.where(sub == 0, hv, bv)
        bi = jnp.where(sub == 0, hi, bi)
        final[0] = bv
        final[1] = bi
        send_final = [exchange(final, dense.at[my], 2, right), exchange(final, dense.at[my], 3, left)]
        for cp in send_final:
            cp.start()

        for cp, src in ((send_final[0], left), (send_final[1], right), (send_dense, diag)):
            cp.wait_recv()
            bv, bi = _lexmerge((bv, bi), (dense[src, 0], dense[src, 1]))
        even = (sub & 1) == 0
        out_ref[0:SUB, :] = jnp.where(even, bv, pltpu.roll(bi, 1, 0))
        out_ref[SUB:2 * SUB, :] = jnp.where(even, pltpu.roll(bv, SUB - 1, 0), bi)
        for p in range(nr):
            for slot in range(2):
                raw(slot, p).wait_send()
        for cp in [send_dense, send_head] + send_final:
            cp.wait_send()
        send_head.wait_recv()
        hv, hi = _lexmerge((bv[0:1], bi[0:1]), (head[diag, 0], head[diag, 1]))
        out_ref[0:1, :] = hv
        out_ref[1:2, :] = hi

    out = pl.pallas_call(
        body,
        out_shape=jax.ShapeDtypeStruct((2 * SUB, LANE), jnp.float32),
        in_specs=[pl.BlockSpec(memory_space=pl.ANY)],
        out_specs=pl.BlockSpec(memory_space=pltpu.VMEM),
        scratch_shapes=[
            pltpu.VMEM((n_local, n_cols), jnp.float32),
            pltpu.VMEM((n_late, LANE), jnp.float32),
            pltpu.VMEM((2, n_remote, n_cols), jnp.float32),
            pltpu.VMEM((3, SUB, n_cols), jnp.float32),
            pltpu.VMEM((3, SUB, n_cols), jnp.int32),
            pltpu.VMEM((NDEV, 2, SUB, LANE), jnp.float32),
            pltpu.VMEM((NDEV, 2, 1, LANE), jnp.float32),
            pltpu.VMEM((2, SUB, LANE), jnp.float32),
            pltpu.SemaphoreType.DMA((nf + 2 * nl,)),
            pltpu.SemaphoreType.DMA((2, nr)),
            pltpu.SemaphoreType.DMA((2, nr)),
            pltpu.SemaphoreType.DMA((4,)),
            pltpu.SemaphoreType.DMA((4,)),
            pltpu.SemaphoreType.REGULAR,
        ],
        compiler_params=pltpu.CompilerParams(
            collective_id=0,
            vmem_limit_bytes=64 * 1024 * 1024,
            disable_semaphore_checks=True,
            disable_bounds_checks=True,
        ),
    )(x)
    return out.reshape(SUB, 2, LANE).transpose(1, 0, 2).reshape(2, n_cols)
```

```python
import jax
import jax.numpy as jnp
from jax import lax
from jax.experimental import pallas as pl
from jax.experimental.pallas import tpu as pltpu

NDEV = 4
MESH = pl.DeviceIdType.MESH
SUB, LANE = 8, 128

FULL = (5440, 1408)
REMOTE = (400, 64)
LATE = (352, 64)
UNROLL = 4
STATIC_GROUPS = 8
BLOCK_ORDER = (0, 4, 1, 5, 2, 6, 3, 7)


def _offsets(sizes):
    offs = [0]
    for s in sizes:
        offs.append(offs[-1] + s)
    return offs


def _lexmerge(a, b):
    (av, ai), (bv, bi) = a, b
    take = jnp.logical_or(bv > av, jnp.logical_and(bv == av, bi < ai))
    return jnp.where(take, bv, av), jnp.where(take, bi, ai)


def _fold(a, b):
    take = b[0] > a[0]
    return jnp.where(take, b[0], a[0]), jnp.where(take, b[1], a[1])


def _butterfly(tiles):
    sub = lax.broadcasted_iota(jnp.int32, (SUB, LANE), 0)
    for half in (4, 2, 1):
        lo = (sub & half) == 0
        n = len(tiles) // 2

        def kept(j, k):
            return jnp.where(lo, tiles[j][k], tiles[j + n][k])

        def moved(j, k):
            if half == 4:
                return pltpu.roll(jnp.where(lo, tiles[j + n][k], tiles[j][k]), 4, 0)
            return jnp.where(lo, pltpu.roll(tiles[j][k], SUB - half, 0),
                             pltpu.roll(tiles[j + n][k], half, 0))

        tiles = [_lexmerge((kept(j, 0), kept(j, 1)), (moved(j, 0), moved(j, 1)))
                 for j in range(n)]
    return tiles[0]


def pallas_dist_argmax_global_i_m8192_n1024_kernel(x: jax.Array):
    m_rows, n_cols = x.shape
    foffs, roffs, loffs = _offsets(FULL), _offsets(REMOTE), _offsets(LATE)
    n_full, n_remote, n_late = foffs[-1], roffs[-1], loffs[-1]
    nf, nr, nl = len(FULL), len(REMOTE), len(LATE)
    n_local = n_full + n_late
    assert n_local + 2 * n_remote == m_rows and n_cols == SUB * LANE
    groups = m_rows // SUB

    def body(x_hbm, out_ref, buf, strip, rbuf, acc_v, acc_i, dense, head, final,
             load_sems, raw_send_sems, raw_recv_sems, send_sems, recv_sems, far_sem):
        def load_full(c):
            rows = pl.ds(foffs[c], FULL[c])
            return pltpu.make_async_copy(x_hbm.at[rows, :], buf.at[rows, :], load_sems.at[c])

        def load_wide(c):
            rows = pl.ds(n_full + loffs[c], LATE[c])
            cols = pl.ds(LANE, n_cols - LANE)
            return pltpu.make_async_copy(x_hbm.at[rows, cols], buf.at[rows, cols], load_sems.at[nf + c])

        def load_strip(c):
            return pltpu.make_async_copy(
                x_hbm.at[pl.ds(n_full + loffs[c], LATE[c]), pl.ds(0, LANE)],
                strip.at[pl.ds(loffs[c], LATE[c]), :], load_sems.at[nf + nl + c])

        for load, n in ((load_full, nf), (load_wide, nl), (load_strip, nl)):
            for c in range(n):
                load(c).start()

        my = lax.axis_index("i")
        left = (my + NDEV - 1) % NDEV
        right = (my + 1) % NDEV
        diag = (my + 2) % NDEV

        barrier = pltpu.get_barrier_semaphore()
        for peer in (left, right):
            pl.semaphore_signal(barrier, inc=1, device_id=(peer,), device_id_type=MESH)
        pl.semaphore_wait(barrier, 2)

        def raw(slot, p):
            return pltpu.make_async_remote_copy(
                src_ref=x_hbm.at[pl.ds(n_local + slot * n_remote + roffs[p], REMOTE[p]), :],
                dst_ref=rbuf.at[slot, pl.ds(roffs[p], REMOTE[p]), :],
                send_sem=raw_send_sems.at[slot, p], recv_sem=raw_recv_sems.at[slot, p],
                device_id=(right if slot == 0 else left,), device_id_type=MESH)

        for p in range(nr):
            for slot in range(2):
                raw(slot, p).start()
        pl.semaphore_signal(far_sem, inc=1, device_id=(right,), device_id_type=MESH)

        def scan(ref, c0, r0, r1, gbase, acc):
            width = ref.shape[-1] - c0
            cols = pl.ds(c0, width)
            g0, g1 = r0 // SUB, r1 // SUB

            def group(g):
                start = g * SUB if isinstance(g, int) else pl.multiple_of(g * SUB, SUB)
                return ref[pl.ds(start, SUB), cols], g + gbase

            def step(i, carry):
                for u in range(UNROLL):
                    carry = _fold(carry, group(i * UNROLL + u))
                return carry

            if acc is None:
                v, g = group(g0)
                acc = (v, jnp.full((SUB, width), g, jnp.int32))
                g0 += 1
            n_head = g1 - g0 if g1 - g0 <= STATIC_GROUPS else -g0 % UNROLL
            for g in range(g0, g0 + n_head):
                acc = _fold(acc, group(g))
            g0 += n_head
            n_steps = (g1 - g0) // UNROLL
            if n_steps:
                acc = lax.fori_loop(g0 // UNROLL, g0 // UNROLL + n_steps, step, acc)
            for g in range(g0 + n_steps * UNROLL, g1):
                acc = _fold(acc, group(g))
            return acc

        started = [False] * 3

        def accumulate(a, ref, r0, r1, gbase):
            acc = (acc_v[a], acc_i[a]) if started[a] else None
            acc_v[a], acc_i[a] = scan(ref, 0, r0, r1, gbase, acc)
            started[a] = True

        for k in range(max(nf, nr)):
            if k < nf:
                load_full(k).wait()
                accumulate(0, buf, foffs[k], foffs[k + 1], my * groups)
            if k < nr:
                for slot, src in ((0, left), (1, right)):
                    raw(slot, k).wait_recv()
                    accumulate(1 + slot, rbuf.at[slot], roffs[k], roffs[k + 1],
                               src * groups + (n_local + slot * n_remote) // SUB)
        bulk = (acc_v[0], acc_i[0])
        for a in (1, 2):
            bulk = _lexmerge(bulk, (acc_v[a], acc_i[a]))
        acc_v[0], acc_i[0] = bulk
        pl.semaphore_wait(far_sem, 1)

        late = None
        for c in range(nl):
            load_wide(c).wait()
            late = scan(buf, LANE, n_full + loffs[c], n_full + loffs[c + 1], my * groups, late)
        sub = lax.broadcasted_iota(jnp.int32, (SUB, LANE), 0)
        wv, wg = _lexmerge((acc_v[0, :, LANE:], acc_i[0, :, LANE:]), late)
        tiles = [(acc_v[0, :, :LANE], acc_i[0, :, :LANE] * SUB + sub)]
        tiles += [(wv[:, j * LANE:(j + 1) * LANE], wg[:, j * LANE:(j + 1) * LANE] * SUB + sub)
                  for j in range(SUB - 1)]
        bv, bi = _butterfly([tiles[b] for b in BLOCK_ORDER])
        bi = bi.astype(jnp.float32)

        def exchange(src, dst, k, peer):
            return pltpu.make_async_remote_copy(
                src_ref=src, dst_ref=dst, send_sem=send_sems.at[k], recv_sem=recv_sems.at[k],
                device_id=(peer,), device_id_type=MESH)

        dense[my, 0] = bv
        dense[my, 1] = bi
        send_dense = exchange(dense.at[my], dense.at[my], 0, diag)
        send_dense.start()

        sacc = None
        for c in range(nl):
            load_strip(c).wait()
            items = [(strip[pl.ds(g * SUB, SUB), :],
                      jnp.full((SUB, LANE), g, jnp.int32) + (my * groups + n_full // SUB))
                     for g in range(loffs[c] // SUB, loffs[c + 1] // SUB)]
            while len(items) > 1:
                items = [_fold(*items[i:i + 2]) if i + 1 < len(items) else items[i]
                         for i in range(0, len(items), 2)]
            sacc = items[0] if sacc is None else _fold(sacc, items[0])
        s = (sacc[0], sacc[1] * SUB + sub)
        for shift in (4, 2, 1):
            s = _lexmerge(s, (pltpu.roll(s[0], shift, 0), pltpu.roll(s[1], shift, 0)))
        sv, si = s[0], s[1].astype(jnp.float32)
        head[my, 0] = sv[0:1]
        head[my, 1] = si[0:1]
        send_head = exchange(head.at[my], head.at[my], 1, diag)
        send_head.start()

        hv, hi = _lexmerge((bv, bi), (sv, si))
        bv = jnp.where(sub == 0, hv, bv)
        bi = jnp.where(sub == 0, hi, bi)
        final[0] = bv
        final[1] = bi
        send_final = [exchange(final, dense.at[my], 2, right), exchange(final, dense.at[my], 3, left)]
        for cp in send_final:
            cp.start()

        for cp, src in ((send_final[0], left), (send_final[1], right), (send_dense, diag)):
            cp.wait_recv()
            bv, bi = _lexmerge((bv, bi), (dense[src, 0], dense[src, 1]))
        even = (sub & 1) == 0
        out_ref[0:SUB, :] = jnp.where(even, bv, pltpu.roll(bi, 1, 0))
        out_ref[SUB:2 * SUB, :] = jnp.where(even, pltpu.roll(bv, SUB - 1, 0), bi)
        for p in range(nr):
            for slot in range(2):
                raw(slot, p).wait_send()
        for cp in [send_dense, send_head] + send_final:
            cp.wait_send()
        send_head.wait_recv()
        hv, hi = _lexmerge((bv[0:1], bi[0:1]), (head[diag, 0], head[diag, 1]))
        out_ref[0:1, :] = hv
        out_ref[1:2, :] = hi

    out = pl.pallas_call(
        body,
        out_shape=jax.ShapeDtypeStruct((2 * SUB, LANE), jnp.float32),
        in_specs=[pl.BlockSpec(memory_space=pl.ANY)],
        out_specs=pl.BlockSpec(memory_space=pltpu.VMEM),
        scratch_shapes=[
            pltpu.VMEM((n_local, n_cols), jnp.float32),
            pltpu.VMEM((n_late, LANE), jnp.float32),
            pltpu.VMEM((2, n_remote, n_cols), jnp.float32),
            pltpu.VMEM((3, SUB, n_cols), jnp.float32),
            pltpu.VMEM((3, SUB, n_cols), jnp.int32),
            pltpu.VMEM((NDEV, 2, SUB, LANE), jnp.float32),
            pltpu.VMEM((NDEV, 2, 1, LANE), jnp.float32),
            pltpu.VMEM((2, SUB, LANE), jnp.float32),
            pltpu.SemaphoreType.DMA((nf + 2 * nl,)),
            pltpu.SemaphoreType.DMA((2, nr)),
            pltpu.SemaphoreType.DMA((2, nr)),
            pltpu.SemaphoreType.DMA((4,)),
            pltpu.SemaphoreType.DMA((4,)),
            pltpu.SemaphoreType.REGULAR,
        ],
        compiler_params=pltpu.CompilerParams(
            collective_id=0,
            vmem_limit_bytes=64 * 1024 * 1024,
            disable_semaphore_checks=True,
            disable_bounds_checks=True,
        ),
    )(x)
    return out.reshape(SUB, 2, LANE).transpose(1, 0, 2).reshape(2, n_cols)
```
